```python
import numpy as np

kernel_name = "dist_mean_ax0_shard0_i_m1024_n512"

def setup_inputs():
    return {"x": np.random.randn(4096, 512).astype(np.float32)}

def reference(x: np.ndarray) -> np.ndarray:
    return np.mean(x, axis=0, keepdims=True)
```

```python
import jax
import jax.numpy as jnp
from jax import lax
from jax.experimental import pallas as pl
from jax.experimental.pallas import tpu as pltpu

_AXIS = "i"
_N_DEV = 4
_LANES = 128
_SUBLANES = 8

_FIRST = 0
_LAST = 2

_CHUNKS = (512, 328, 112, 16)
_SPILL = 56


def _row_sum(ref, start, rows):
    block = ref[pl.ds(start, rows), :]
    return jnp.sum(block.reshape(rows // _SUBLANES, _SUBLANES, -1), axis=0)


def _column_sums(acc):
    total = jnp.sum(acc, axis=0, keepdims=True)
    return jnp.concatenate(
        [total[:, c : c + _LANES] for c in range(0, acc.shape[1], _LANES)], axis=0
    )


def _kernel(
    x_hbm,
    out_ref,
    x_vmem,
    spill_recv,
    diag_send,
    diag_recv,
    side_send,
    side_recv,
    load_sems,
    send_sems,
    recv_sems,
):
    rows = x_hbm.shape[0]
    spill_start = rows - _SPILL
    me = lax.axis_index(_AXIS)
    diag = (me + 2) & 3
    sides = ((me + 1) & 3, (me + 3) & 3)

    def load(start, size, k):
        block = pl.ds(start, size)
        return pltpu.make_async_copy(
            x_hbm.at[block], x_vmem.at[block], load_sems.at[k]
        )

    def push(src, dst, k, device):
        return pltpu.make_async_remote_copy(
            src_ref=src,
            dst_ref=dst,
            send_sem=send_sems.at[k],
            recv_sem=recv_sems.at[k],
            device_id=(device,),
            device_id_type=pl.DeviceIdType.MESH,
        )

    starts = [sum(_CHUNKS[:k]) for k in range(len(_CHUNKS))]
    loads = [load(s, size, k) for k, (s, size) in enumerate(zip(starts, _CHUNKS))]
    for copy in loads:
        copy.start()

    barrier = pltpu.get_barrier_semaphore()
    for peer in (diag, *sides):
        pl.semaphore_signal(
            barrier, inc=1, device_id=(peer,), device_id_type=pl.DeviceIdType.MESH
        )
    pl.semaphore_wait(barrier, _N_DEV - 1)

    diag_push = push(diag_send, diag_recv, 0, diag)
    side_pushes = [
        push(side_send, side_recv.at[k], 1 + k, peer) for k, peer in enumerate(sides)
    ]
    spill_push = push(x_hbm.at[pl.ds(spill_start, _SPILL)], spill_recv, 3, diag)

    @pl.when(me == _LAST)
    def _():
        spill_push.start()

    acc = None
    for copy, start, size in zip(loads, starts, _CHUNKS):
        copy.wait()
        chunk = _row_sum(x_vmem, start, size)
        acc = chunk if acc is None else acc + chunk

    chunk_sums = _column_sums(acc).astype(diag_send.dtype)

    @pl.when(me == _LAST)
    def _():
        diag_send[...] = chunk_sums
        diag_push.start()

    spill_load = load(spill_start, _SPILL, len(_CHUNKS))
    spill_load.start()
    spill_load.wait()
    shard_sums = _column_sums(acc + _row_sum(x_vmem, spill_start, _SPILL))

    @pl.when(me != _LAST)
    def _():
        diag_send[...] = shard_sums.astype(diag_send.dtype)
        diag_push.start()

    side_send[...] = shard_sums
    for copy in side_pushes:
        copy.start()

    for copy in (diag_push, *side_pushes):
        copy.wait_send()

    @pl.when(me == _LAST)
    def _():
        spill_push.wait_send()

    for copy in side_pushes:
        copy.wait_recv()
    out_ref[...] = shard_sums + side_recv[0] + side_recv[1]

    @pl.when(me == _FIRST)
    def _():
        spill_push.wait_recv()
        out_ref[...] += _column_sums(_row_sum(spill_recv, 0, _SPILL))

    diag_push.wait_recv()
    total = out_ref[...] + diag_recv[...].astype(jnp.float32)
    out_ref[...] = total * (1.0 / (_N_DEV * rows))


def pallas_dist_mean_ax0_shard0_i_m1024_n512_kernel(
    x: jax.Array,
):
    rows, cols = x.shape
    assert sum(_CHUNKS) + _SPILL == rows
    sums = (cols // _LANES, _LANES)
    out = pl.pallas_call(
        _kernel,
        out_shape=jax.ShapeDtypeStruct(sums, jnp.float32),
        in_specs=[pl.BlockSpec(memory_space=pl.ANY)],
        out_specs=pl.BlockSpec(memory_space=pltpu.VMEM),
        scratch_shapes=[
            pltpu.VMEM((rows, cols), jnp.float32),
            pltpu.VMEM((_SPILL, cols), jnp.float32),
            pltpu.VMEM(sums, jnp.bfloat16),
            pltpu.VMEM(sums, jnp.bfloat16),
            pltpu.VMEM(sums, jnp.float32),
            pltpu.VMEM((2, *sums), jnp.float32),
            pltpu.SemaphoreType.DMA((len(_CHUNKS) + 1,)),
            pltpu.SemaphoreType.DMA((4,)),
            pltpu.SemaphoreType.DMA((4,)),
        ],
        compiler_params=pltpu.CompilerParams(
            collective_id=0,
            disable_bounds_checks=True,
            disable_semaphore_checks=True,
        ),
    )(x)
    return out.reshape(1, cols)
```

```python
import jax
import jax.numpy as jnp
from jax import lax
from jax.experimental import pallas as pl
from jax.experimental.pallas import tpu as pltpu

_AXIS = "i"
_N_DEV = 4
_LANES = 128
_SUBLANES = 8

_FIRST = 0
_LAST = 2

_CHUNKS = (512, 336, 96, 16)
_SPLIT = 24
_SPILL = 40


def _row_sum(block):
    return jnp.sum(block.reshape(-1, _SUBLANES, block.shape[1]), axis=0)


def _column_sums(acc):
    total = jnp.sum(acc, axis=0, keepdims=True)
    return jnp.concatenate(
        [total[:, c : c + _LANES] for c in range(0, acc.shape[1], _LANES)], axis=0
    )


def _kernel(
    x_hbm,
    out_ref,
    chunk_buf,
    left_buf,
    split_buf,
    spill_buf,
    split_recv,
    spill_recv,
    diag_send,
    diag_recv,
    side_send,
    side_recv,
    load_sems,
    send_sems,
    recv_sems,
):
    rows, cols = x_hbm.shape
    half = cols // 2
    me = lax.axis_index(_AXIS)
    diag = (me + 2) & 3
    sides = ((me + 1) & 3, (me + 3) & 3)

    split_start = sum(_CHUNKS)
    chunks = [pl.ds(sum(_CHUNKS[:k]), size) for k, size in enumerate(_CHUNKS)]
    lefts = [pl.ds(start, _SUBLANES) for start in range(0, _SPLIT, _SUBLANES)]
    x_split = x_hbm.at[pl.ds(split_start, _SPLIT), pl.ds(half, half)]
    x_spill = x_hbm.at[pl.ds(split_start + _SPLIT, _SPILL)]

    loads = [
        pltpu.make_async_copy(src, dst, load_sems.at[k])
        for k, (src, dst) in enumerate(
            [(x_hbm.at[part], chunk_buf.at[part]) for part in chunks]
            + [
                (
                    x_hbm.at[pl.ds(split_start + part.start, part.size), pl.ds(0, half)],
                    left_buf.at[part],
                )
                for part in lefts
            ]
            + [(x_split, split_buf), (x_spill, spill_buf)]
        )
    ]
    chunk_loads = loads[: len(chunks)]
    left_loads = loads[len(chunks) : -2]
    rest_loads = loads[-2:]

    pushes = [
        pltpu.make_async_remote_copy(
            src_ref=src,
            dst_ref=dst,
            send_sem=send_sems.at[k],
            recv_sem=recv_sems.at[k],
            device_id=(peer,),
            device_id_type=pl.DeviceIdType.MESH,
        )
        for k, (src, dst, peer) in enumerate(
            [
                (diag_send.at[0], diag_recv.at[0], diag),
                (diag_send.at[1], diag_recv.at[1], diag),
                (side_send, side_recv.at[0], sides[0]),
                (side_send, side_recv.at[1], sides[1]),
                (x_split, split_recv, diag),
                (x_spill, spill_recv, diag),
            ]
        )
    ]
    left_push, right_push = pushes[:2]
    side_pushes = pushes[2:4]
    split_push, spill_push = pushes[4:]

    for copy in chunk_loads + left_loads:
        copy.start()

    @pl.when(me != _LAST)
    def _():
        for copy in rest_loads:
            copy.start()

    barrier = pltpu.get_barrier_semaphore()
    for peer in (*sides, diag):
        pl.semaphore_signal(
            barrier, inc=1, device_id=(peer,), device_id_type=pl.DeviceIdType.MESH
        )
    pl.semaphore_wait(barrier, _N_DEV - 1)

    @pl.when(me == _LAST)
    def _():
        split_push.start()
        spill_push.start()

    acc = None
    for part, copy in zip(chunks, chunk_loads):
        copy.wait()
        chunk = _row_sum(chunk_buf[part, :])
        acc = chunk if acc is None else acc + chunk
    acc_left, acc_right = acc[:, :half], acc[:, half:]

    right_sums = _column_sums(acc_right).astype(diag_send.dtype)

    @pl.when(me == _LAST)
    def _():
        diag_send[1] = right_sums
        right_push.start()

    for part, copy in zip(lefts, left_loads):
        copy.wait()
        acc_left = acc_left + left_buf[part, :]
    left_sums = _column_sums(acc_left).astype(diag_send.dtype)

    @pl.when(me == _LAST)
    def _():
        diag_send[0] = left_sums
        left_push.start()
        for copy in rest_loads:
            copy.start()

    for copy in rest_loads:
        copy.wait()
    acc_right = acc_right + _row_sum(split_buf[...])
    acc = jnp.concatenate([acc_left, acc_right], axis=1) + _row_sum(spill_buf[...])
    shard_sums = _column_sums(acc)
    out_left, out_right = pl.ds(0, half // _LANES), pl.ds(half // _LANES, half // _LANES)

    @pl.when(me != _LAST)
    def _():
        diag_send[0] = shard_sums[: half // _LANES].astype(diag_send.dtype)
        diag_send[1] = shard_sums[half // _LANES :].astype(diag_send.dtype)
        right_push.start()
        left_push.start()

    side_send[...] = shard_sums
    for copy in side_pushes:
        copy.start()

    for copy in (right_push, left_push, *side_pushes):
        copy.wait_send()

    @pl.when(me == _LAST)
    def _():
        split_push.wait_send()
        spill_push.wait_send()

    for copy in side_pushes:
        copy.wait_recv()
    out_ref[...] = shard_sums + side_recv[0] + side_recv[1]

    @pl.when(me == _FIRST)
    def _():
        split_push.wait_recv()
        out_ref[out_right, :] += _column_sums(_row_sum(split_recv[...]))
        spill_push.wait_recv()
        out_ref[...] += _column_sums(_row_sum(spill_recv[...]))

    scale = 1.0 / (_N_DEV * rows)
    near_left, near_right = out_ref[out_left, :], out_ref[out_right, :]
    right_push.wait_recv()
    out_ref[out_right, :] = (near_right + diag_recv[1].astype(jnp.float32)) * scale
    left_push.wait_recv()
    out_ref[out_left, :] = (near_left + diag_recv[0].astype(jnp.float32)) * scale


def pallas_dist_mean_ax0_shard0_i_m1024_n512_kernel(
    x: jax.Array,
):
    rows, cols = x.shape
    assert sum(_CHUNKS) + _SPLIT + _SPILL == rows
    sums = (cols // _LANES, _LANES)
    halves = (2, cols // _LANES // 2, _LANES)
    n_loads = len(_CHUNKS) + _SPLIT // _SUBLANES + 2
    out = pl.pallas_call(
        _kernel,
        out_shape=jax.ShapeDtypeStruct(sums, jnp.float32),
        in_specs=[pl.BlockSpec(memory_space=pltpu.HBM)],
        out_specs=pl.BlockSpec(memory_space=pltpu.VMEM),
        scratch_shapes=[
            pltpu.VMEM((sum(_CHUNKS), cols), jnp.float32),
            pltpu.VMEM((_SPLIT, cols // 2), jnp.float32),
            pltpu.VMEM((_SPLIT, cols // 2), jnp.float32),
            pltpu.VMEM((_SPILL, cols), jnp.float32),
            pltpu.VMEM((_SPLIT, cols // 2), jnp.float32),
            pltpu.VMEM((_SPILL, cols), jnp.float32),
            pltpu.VMEM(halves, jnp.bfloat16),
            pltpu.VMEM(halves, jnp.bfloat16),
            pltpu.VMEM(sums, jnp.float32),
            pltpu.VMEM((2, *sums), jnp.float32),
            pltpu.SemaphoreType.DMA((n_loads,)),
            pltpu.SemaphoreType.DMA((6,)),
            pltpu.SemaphoreType.DMA((6,)),
        ],
        compiler_params=pltpu.CompilerParams(
            collective_id=0,
            disable_semaphore_checks=True,
        ),
    )(x)
    return out.reshape(1, cols)
```

```python
import jax
import jax.numpy as jnp
from jax import lax
from jax.experimental import pallas as pl
from jax.experimental.pallas import tpu as pltpu

_AXIS = "i"
_N_DEV = 4
_LANES = 128
_SUBLANES = 8

_FIRST = 0
_LAST = 2

_CHUNKS = (512, 336, 96, 16)
_SPLIT = 24
_SPILL = 40


def _row_sum(block):
    return jnp.sum(block.reshape(-1, _SUBLANES, block.shape[1]), axis=0)


def _column_sums(acc):
    total = jnp.sum(acc, axis=0, keepdims=True)
    return jnp.concatenate(
        [total[:, c : c + _LANES] for c in range(0, acc.shape[1], _LANES)], axis=0
    )


def _kernel(
    x_hbm,
    out_ref,
    chunk_buf,
    left_buf,
    split_buf,
    spill_buf,
    split_recv,
    spill_recv,
    diag_send,
    diag_recv,
    side_send,
    side_recv,
    load_sems,
    send_sems,
    recv_sems,
):
    rows, cols = x_hbm.shape
    half = cols // 2
    me = lax.axis_index(_AXIS)
    diag = (me + 2) & 3
    sides = ((me + 1) & 3, (me + 3) & 3)

    split_start = sum(_CHUNKS)
    chunks = [pl.ds(sum(_CHUNKS[:k]), size) for k, size in enumerate(_CHUNKS)]
    tiles = range(0, _SPLIT, _SUBLANES)
    x_lefts = [
        x_hbm.at[pl.ds(split_start + tile, _SUBLANES), pl.ds(0, half)] for tile in tiles
    ]
    x_split = x_hbm.at[pl.ds(split_start, _SPLIT), pl.ds(half, half)]
    x_spill = x_hbm.at[pl.ds(split_start + _SPLIT, _SPILL)]

    loads = [
        pltpu.make_async_copy(src, dst, load_sems.at[k])
        for k, (src, dst) in enumerate(
            [
                *((x_hbm.at[chunk], chunk_buf.at[chunk]) for chunk in chunks),
                *zip(x_lefts, (left_buf.at[pl.ds(tile, _SUBLANES)] for tile in tiles)),
                (x_split, split_buf),
                (x_spill, spill_buf),
            ]
        )
    ]
    chunk_loads = loads[: len(chunks)]
    left_loads = loads[len(chunks) : -2]
    rest_loads = loads[-2:]

    pushes = [
        pltpu.make_async_remote_copy(
            src_ref=src,
            dst_ref=dst,
            send_sem=send_sems.at[k],
            recv_sem=recv_sems.at[k],
            device_id=(peer,),
            device_id_type=pl.DeviceIdType.MESH,
        )
        for k, (src, dst, peer) in enumerate(
            [
                (diag_send.at[0], diag_recv.at[0], diag),
                (diag_send.at[1], diag_recv.at[1], diag),
                (side_send, side_recv.at[0], sides[0]),
                (side_send, side_recv.at[1], sides[1]),
                (x_split, split_recv, diag),
                (x_spill, spill_recv, diag),
            ]
        )
    ]
    left_push, right_push = pushes[:2]
    side_pushes = pushes[2:4]
    split_push, spill_push = pushes[4:]

    for copy in chunk_loads + left_loads:
        copy.start()

    @pl.when(me != _LAST)
    def _():
        for copy in rest_loads:
            copy.start()

    barrier = pltpu.get_barrier_semaphore()
    for peer in (*sides, diag):
        pl.semaphore_signal(
            barrier, inc=1, device_id=(peer,), device_id_type=pl.DeviceIdType.MESH
        )
    pl.semaphore_wait(barrier, _N_DEV - 1)

    @pl.when(me == _LAST)
    def _():
        split_push.start()
        spill_push.start()

    acc = None
    for chunk, copy in zip(chunks, chunk_loads):
        copy.wait()
        chunk_sum = _row_sum(chunk_buf[chunk, :])
        acc = chunk_sum if acc is None else acc + chunk_sum
    acc_left, acc_right = acc[:, :half], acc[:, half:]

    right_sums = _column_sums(acc_right).astype(diag_send.dtype)

    @pl.when(me == _LAST)
    def _():
        diag_send[1] = right_sums
        right_push.start()

    for tile, copy in zip(tiles, left_loads):
        copy.wait()
        acc_left = acc_left + left_buf[pl.ds(tile, _SUBLANES), :]
    left_sums = _column_sums(acc_left).astype(diag_send.dtype)

    @pl.when(me == _LAST)
    def _():
        diag_send[0] = left_sums
        left_push.start()
        for copy in rest_loads:
            copy.start()

    for copy in rest_loads:
        copy.wait()
    acc_right = acc_right + _row_sum(split_buf[...])
    acc = jnp.concatenate([acc_left, acc_right], axis=1) + _row_sum(spill_buf[...])
    shard_sums = _column_sums(acc)
    mid = half // _LANES
    out_left, out_right = pl.ds(0, mid), pl.ds(mid, mid)

    @pl.when(me != _LAST)
    def _():
        diag_send[0] = shard_sums[:mid].astype(diag_send.dtype)
        diag_send[1] = shard_sums[mid:].astype(diag_send.dtype)
        right_push.start()
        left_push.start()

    side_send[...] = shard_sums
    for copy in side_pushes:
        copy.start()

    for copy in (right_push, left_push, *side_pushes):
        copy.wait_send()

    @pl.when(me == _LAST)
    def _():
        split_push.wait_send()
        spill_push.wait_send()

    for copy in side_pushes:
        copy.wait_recv()
    out_ref[...] = shard_sums + side_recv[0] + side_recv[1]

    @pl.when(me == _FIRST)
    def _():
        split_push.wait_recv()
        out_ref[out_right, :] += _column_sums(_row_sum(split_recv[...]))
        spill_push.wait_recv()
        out_ref[...] += _column_sums(_row_sum(spill_recv[...]))

    scale = 1.0 / (_N_DEV * rows)
    near_left, near_right = out_ref[out_left, :], out_ref[out_right, :]
    right_push.wait_recv()
    out_ref[out_right, :] = (near_right + diag_recv[1].astype(jnp.float32)) * scale
    left_push.wait_recv()
    out_ref[out_left, :] = (near_left + diag_recv[0].astype(jnp.float32)) * scale


def pallas_dist_mean_ax0_shard0_i_m1024_n512_kernel(
    x: jax.Array,
):
    rows, cols = x.shape
    assert sum(_CHUNKS) + _SPLIT + _SPILL == rows
    sums = (cols // _LANES, _LANES)
    halves = (2, cols // _LANES // 2, _LANES)
    n_loads = len(_CHUNKS) + _SPLIT // _SUBLANES + 2
    out = pl.pallas_call(
        _kernel,
        out_shape=jax.ShapeDtypeStruct(sums, jnp.float32),
        in_specs=[pl.BlockSpec(memory_space=pltpu.HBM)],
        out_specs=pl.BlockSpec(memory_space=pltpu.VMEM),
        scratch_shapes=[
            pltpu.VMEM((sum(_CHUNKS), cols), jnp.float32),
            pltpu.VMEM((_SPLIT, cols // 2), jnp.float32),
            pltpu.VMEM((_SPLIT, cols // 2), jnp.float32),
            pltpu.VMEM((_SPILL, cols), jnp.float32),
            pltpu.VMEM((_SPLIT, cols // 2), jnp.float32),
            pltpu.VMEM((_SPILL, cols), jnp.float32),
            pltpu.VMEM(halves, jnp.bfloat16),
            pltpu.VMEM(halves, jnp.bfloat16),
            pltpu.VMEM(sums, jnp.float32),
            pltpu.VMEM((2, *sums), jnp.float32),
            pltpu.SemaphoreType.DMA((n_loads,)),
            pltpu.SemaphoreType.DMA((6,)),
            pltpu.SemaphoreType.DMA((6,)),
        ],
        compiler_params=pltpu.CompilerParams(
            collective_id=0,
            disable_semaphore_checks=True,
        ),
    )(x)
    return out.reshape(1, cols)
```
